```python
import numpy as np

kernel_name = "dist_ag_xy_y_m1024_n512"

def setup_inputs():
    return {"x": np.random.randn(2048, 512).astype(np.float32)}

def reference(x: np.ndarray) -> np.ndarray:
    return x
```

```python
import jax
import jax.numpy as jnp
from jax import lax
from jax.experimental import pallas as pl
from jax.experimental.pallas import tpu as pltpu

_ROWS, _LANES = 16, 128
_FWD_TILES = 118
_QUEUE_DEPTH = 48
_LOAD_ROWS = (16, 48, 160, 160)
_REST_FROM = 24


def pallas_dist_ag_xy_y_m1024_n512_kernel(x: jax.Array):
    m, n = x.shape
    n_blocks, per_block = m // _ROWS, n // _LANES
    fwd = _FWD_TILES
    full, part = divmod(fwd, per_block)
    assert part > 0 and 2 * (full + 1) < n_blocks
    sent_rows = (n_blocks - full) * _ROWS
    rest_blocks = full
    load_rows = [*_LOAD_ROWS, sent_rows - sum(_LOAD_ROWS), m - sent_rows]
    load_starts = [sum(load_rows[:i]) for i in range(len(load_rows))]
    n_loads = len(load_rows)

    def body(x_ref, o_ref, xin, load_sem, y_send, y_recv, mid_recv, x_send, x_recv,
             ready):
        mx, my = lax.axis_index("x"), lax.axis_index("y")
        y_dev, x_dev = (mx, 1 - my), (1 - mx, my)
        is_00 = jnp.logical_and(mx == 0, my == 0)
        is_10 = jnp.logical_and(mx == 1, my == 0)

        def signal(sem, dev):
            pl.semaphore_signal(sem, inc=1, device_id=dev,
                                device_id_type=pl.DeviceIdType.MESH)

        def remote(ref, send_sem, recv_sem, dev):
            return pltpu.make_async_remote_copy(
                ref, ref, send_sem, recv_sem, device_id=dev,
                device_id_type=pl.DeviceIdType.MESH)

        def rows(start, size, shard=0, col=mx):
            first = jnp.where(col == 0, start, m - start - size)
            return pl.ds(pl.multiple_of(shard * m + first, _ROWS), size)

        def tile(t, shard):
            b, c = divmod(t, per_block)
            return o_ref.at[rows(b * _ROWS, _ROWS, shard), pl.ds(c * _LANES, _LANES)]

        done, todo = pl.ds(0, part * _LANES), pl.ds(part * _LANES, n - part * _LANES)

        def middle(shard):
            lo, hi = full * _ROWS, (n_blocks - 1 - full) * _ROWS
            return [
                remote(o_ref.at[rows(lo, _ROWS, shard), todo],
                       y_send.at[0], mid_recv.at[0], y_dev),
                remote(o_ref.at[rows(lo + _ROWS, hi - lo - _ROWS, shard)],
                       y_send.at[0], mid_recv.at[1], y_dev),
                remote(o_ref.at[rows(hi, _ROWS, shard), todo],
                       y_send.at[1], mid_recv.at[2], y_dev),
            ]

        loads = [
            pltpu.make_async_copy(x_ref.at[rows(s, k)], xin.at[rows(s, k)],
                                  load_sem.at[i])
            for i, (s, k) in enumerate(zip(load_starts, load_rows))
        ]

        barrier = pltpu.get_barrier_semaphore()
        loads[0].start()
        signal(barrier, y_dev)
        pl.when(is_10)(lambda: signal(barrier, x_dev))
        for load in loads[1:]:
            load.start()

        waited = cast = 0

        def cast_up_to(end):
            nonlocal waited, cast
            if end <= cast:
                return
            while waited < n_loads and load_starts[waited] < end:
                loads[waited].wait()
                waited += 1
            o_ref[rows(cast, end - cast, my), :] = (
                xin[rows(cast, end - cast), :].astype(o_ref.dtype))
            cast = end

        def send_y(t):
            if t < fwd:
                cast_up_to((t // per_block + 1) * _ROWS)
                if t == 0:
                    pl.when(is_00)(lambda: pl.semaphore_wait(barrier, 2))
                    pl.when(jnp.logical_not(is_00))(
                        lambda: pl.semaphore_wait(barrier, 1))
                remote(tile(t, my), y_send.at[0], y_recv.at[t], y_dev).start()
                if t == 0:
                    pl.when(is_00)(lambda: signal(ready, (1, 0)))
                if t == 2:

                    @pl.when(is_10)
                    def _():
                        pl.semaphore_wait(ready, 1)
                        signal(ready, (0, 1))
                        signal(ready, (1, 1))

            elif t == fwd:
                cast_up_to(sent_rows)
                for copy in middle(my):
                    copy.start()

        for t in range(_QUEUE_DEPTH):
            send_y(t)
        pl.when(my == 1)(lambda: pl.semaphore_wait(ready, 1))

        for t in range(fwd):
            landed = tile(t, 1 - my)
            remote(landed, y_send.at[0], y_recv.at[t], y_dev).wait_recv()
            s = int(t >= full * per_block)
            remote(landed, x_send.at[s], x_recv.at[s], x_dev).start()
            send_y(_QUEUE_DEPTH + t)
            if t >= max(_REST_FROM, fwd - _QUEUE_DEPTH + 1):
                steps = fwd - max(_REST_FROM, fwd - _QUEUE_DEPTH + 1)
                k = t + 1 - (fwd - steps)
                cast_up_to(sent_rows + (k * rest_blocks // steps) * _ROWS)
        assert cast == m and waited == n_loads

        hi = (n_blocks - 1 - full) * _ROWS
        remote(o_ref.at[rows(0, hi, my)], y_send.at[0], mid_recv.at[0], y_dev).wait_send()
        remote(o_ref.at[rows(hi, _ROWS, my), todo],
               y_send.at[1], mid_recv.at[0], y_dev).wait_send()
        for col, wait in ((mx, "send"), (1 - mx, "recv")):
            blocks = o_ref.at[rows(0, full * _ROWS, 1 - my, col)]
            tiles = o_ref.at[rows(full * _ROWS, _ROWS, 1 - my, col), done]
            if wait == "recv":
                for copy in middle(1 - my):
                    copy.wait_recv()
            for s, region in enumerate((blocks, tiles)):
                copy = remote(region, x_send.at[s], x_recv.at[s], x_dev)
                copy.wait_send() if wait == "send" else copy.wait_recv()

    dma = pltpu.SemaphoreType.DMA
    return pl.pallas_call(
        body,
        out_shape=jax.ShapeDtypeStruct((2 * m, n), jnp.bfloat16),
        in_specs=[pl.BlockSpec(memory_space=pltpu.HBM)],
        out_specs=pl.BlockSpec(memory_space=pltpu.VMEM),
        scratch_shapes=[
            pltpu.VMEM((m, n), x.dtype),
            dma((n_loads,)),
            dma((2,)),
            dma((fwd,)),
            dma((3,)),
            dma((2,)),
            dma((2,)),
            pltpu.SemaphoreType.REGULAR,
        ],
        compiler_params=pltpu.CompilerParams(
            collective_id=0, disable_semaphore_checks=True),
    )(x)
```
